```python
import numpy as np

kernel_name = "dist_argmax_global_i_m4096_n1024"

def setup_inputs():
    return {"x": np.random.randn(16384, 1024).astype(np.float32)}

def reference(x: np.ndarray) -> np.ndarray:
    idx = np.argmax(x, axis=0).astype(np.float32)
    val = np.max(x, axis=0)
    return np.stack([val, idx], axis=0)
```

```python
import jax
import jax.numpy as jnp
from jax import lax
from jax.experimental import pallas as pl
from jax.experimental.pallas import tpu as pltpu

N_DEV = 4
BR = 512
UNROLL = 8


def pallas_dist_argmax_global_i_m4096_n1024_kernel(x):
    m_per, n = x.shape
    nsteps = m_per // BR
    groups = BR // 8

    def body(x_ref, out_ref, m_acc, i_acc, comm, send_sems, recv_sems):
        step = pl.program_id(0)
        my = lax.axis_index("i")

        @pl.when(step == 0)
        def _():
            barrier = pltpu.get_barrier_semaphore()
            for d in range(1, N_DEV):
                pl.semaphore_signal(
                    barrier, inc=1, device_id=((my + d) % N_DEV,),
                    device_id_type=pl.DeviceIdType.MESH)
            m_acc[...] = jnp.full(m_acc.shape, -jnp.inf, jnp.float32)
            i_acc[...] = jnp.zeros(i_acc.shape, jnp.int32)

        base = step * groups

        def loop(g, carry):
            m, idx = carry
            xg = x_ref[pl.ds(pl.multiple_of(g * 8, 8), 8), :]
            gt = xg > m
            return jnp.where(gt, xg, m), jnp.where(gt, base + g, idx)

        m, idx = lax.fori_loop(0, groups, loop, (m_acc[...], i_acc[...]),
                               unroll=UNROLL)
        m_acc[...] = m
        i_acc[...] = idx

        @pl.when(step == nsteps - 1)
        def _():
            mm = jnp.max(m, axis=0, keepdims=True)
            sub = lax.broadcasted_iota(jnp.int32, m.shape, 0)
            rows = jnp.where(m == mm, idx * 8 + sub, jnp.int32(2 ** 30))
            rmin = jnp.min(rows, axis=0, keepdims=True) + my * m_per
            comm[my, 0:1, :] = mm
            comm[my, 1:2, :] = rmin.astype(jnp.float32)

            barrier = pltpu.get_barrier_semaphore()
            pl.semaphore_wait(barrier, N_DEV - 1)

            copies = []
            for d in range(1, N_DEV):
                tgt = (my + d) % N_DEV
                cp = pltpu.make_async_remote_copy(
                    src_ref=comm.at[my], dst_ref=comm.at[my],
                    send_sem=send_sems.at[d - 1],
                    recv_sem=recv_sems.at[d - 1],
                    device_id=(tgt,), device_id_type=pl.DeviceIdType.MESH)
                cp.start()
                copies.append(cp)
            for d in range(1, N_DEV):
                src = (my - d) % N_DEV
                rc = pltpu.make_async_remote_copy(
                    src_ref=comm.at[src], dst_ref=comm.at[src],
                    send_sem=send_sems.at[d - 1],
                    recv_sem=recv_sems.at[d - 1],
                    device_id=(src,), device_id_type=pl.DeviceIdType.MESH)
                rc.wait_recv()
            for cp in copies:
                cp.wait_send()

            bv = comm[0, 0:1, :]
            bi = comm[0, 1:2, :]
            for j in range(1, N_DEV):
                v = comm[j, 0:1, :]
                gt = v > bv
                bi = jnp.where(gt, comm[j, 1:2, :], bi)
                bv = jnp.where(gt, v, bv)
            out_ref[0:1, :] = bv
            out_ref[1:2, :] = bi

    return pl.pallas_call(
        body,
        out_shape=jax.ShapeDtypeStruct((2, n), jnp.float32),
        grid=(nsteps,),
        in_specs=[pl.BlockSpec((BR, n), lambda i: (i, 0))],
        out_specs=pl.BlockSpec((2, n), lambda i: (0, 0)),
        scratch_shapes=[
            pltpu.VMEM((8, n), jnp.float32),
            pltpu.VMEM((8, n), jnp.int32),
            pltpu.VMEM((N_DEV, 2, n), jnp.float32),
            pltpu.SemaphoreType.DMA((N_DEV - 1,)),
            pltpu.SemaphoreType.DMA((N_DEV - 1,)),
        ],
        compiler_params=pltpu.CompilerParams(
            collective_id=0, dimension_semantics=("arbitrary",)),
    )(x)
```

```python
import jax
import jax.numpy as jnp
from jax import lax
from jax.experimental import pallas as pl
from jax.experimental.pallas import tpu as pltpu

N_DEV = 4
UNROLL = 8


def _chunk_rows(m_per):
    big = 512
    if m_per % big or m_per < 2 * big:
        return [m_per]
    return [big] * (m_per // big - 1) + [256, 128, 64, 32, 16, 16]


def _better(v, bv):
    return jnp.logical_and(jnp.logical_not(v <= bv), bv == bv)


def pallas_dist_argmax_global_i_m4096_n1024_kernel(x):
    m_per, n = x.shape
    chunks = _chunk_rows(m_per)
    offs = [sum(chunks[:c]) for c in range(len(chunks))]

    def body(x_hbm, out_ref, buf, comm, in_sems, send_sems, recv_sems):
        my = lax.axis_index("i")

        barrier = pltpu.get_barrier_semaphore()
        for d in range(1, N_DEV):
            pl.semaphore_signal(
                barrier, inc=1, device_id=((my + d) % N_DEV,),
                device_id_type=pl.DeviceIdType.MESH)

        def load(c):
            return pltpu.make_async_copy(
                x_hbm.at[pl.ds(offs[c], chunks[c])],
                buf.at[pl.ds(offs[c], chunks[c])], in_sems.at[c])

        for c in range(len(chunks)):
            load(c).start()

        def loop(g, carry):
            m, idx = carry
            xg = buf[pl.ds(pl.multiple_of(g * 8, 8), 8), :]
            gt = _better(xg, m)
            return jnp.where(gt, xg, m), jnp.where(gt, g, idx)

        m = jnp.full((8, n), -jnp.inf, jnp.float32)
        idx = jnp.zeros((8, n), jnp.int32)
        for c in range(len(chunks)):
            load(c).wait()
            g0 = offs[c] // 8
            m, idx = lax.fori_loop(g0, g0 + chunks[c] // 8, loop, (m, idx),
                                   unroll=min(UNROLL, chunks[c] // 8))

        rows = idx * 8 + lax.broadcasted_iota(jnp.int32, m.shape, 0)
        bv, br = m[0:1, :], rows[0:1, :]
        for s in range(1, 8):
            v, r = m[s:s + 1, :], rows[s:s + 1, :]
            tie = jnp.logical_or(v == bv, jnp.logical_and(v != v, bv != bv))
            take = jnp.logical_or(_better(v, bv),
                                  jnp.logical_and(tie, r < br))
            bv, br = jnp.where(take, v, bv), jnp.where(take, r, br)
        comm[my, 0:1, :] = bv
        comm[my, 1:2, :] = (br + my * m_per).astype(jnp.float32)

        pl.semaphore_wait(barrier, N_DEV - 1)
        sends = []
        for d in range(1, N_DEV):
            cp = pltpu.make_async_remote_copy(
                src_ref=comm.at[my], dst_ref=comm.at[my],
                send_sem=send_sems.at[d - 1], recv_sem=recv_sems.at[d - 1],
                device_id=((my + d) % N_DEV,),
                device_id_type=pl.DeviceIdType.MESH)
            cp.start()
            sends.append(cp)
        for d in range(1, N_DEV):
            src = (my - d) % N_DEV
            pltpu.make_async_remote_copy(
                src_ref=comm.at[src], dst_ref=comm.at[src],
                send_sem=send_sems.at[d - 1], recv_sem=recv_sems.at[d - 1],
                device_id=(src,),
                device_id_type=pl.DeviceIdType.MESH).wait_recv()
        for cp in sends:
            cp.wait_send()

        bv, bi = comm[0, 0:1, :], comm[0, 1:2, :]
        for j in range(1, N_DEV):
            v = comm[j, 0:1, :]
            take = _better(v, bv)
            bi = jnp.where(take, comm[j, 1:2, :], bi)
            bv = jnp.where(take, v, bv)
        out_ref[0:1, :] = bv
        out_ref[1:2, :] = bi

    return pl.pallas_call(
        body,
        out_shape=jax.ShapeDtypeStruct((2, n), jnp.float32),
        in_specs=[pl.BlockSpec(memory_space=pl.ANY)],
        out_specs=pl.BlockSpec(memory_space=pltpu.VMEM),
        scratch_shapes=[
            pltpu.VMEM((m_per, n), jnp.float32),
            pltpu.VMEM((N_DEV, 2, n), jnp.float32),
            pltpu.SemaphoreType.DMA((len(chunks),)),
            pltpu.SemaphoreType.DMA((N_DEV - 1,)),
            pltpu.SemaphoreType.DMA((N_DEV - 1,)),
        ],
        compiler_params=pltpu.CompilerParams(
            collective_id=0, vmem_limit_bytes=64 * 1024 * 1024),
    )(x)
```

```python
import jax
import jax.numpy as jnp
from jax import lax
from jax.experimental import pallas as pl
from jax.experimental.pallas import tpu as pltpu

N_DEV = 4
UNROLL = 8


def _chunk_rows(m_per):
    big = 512
    if m_per % big or m_per < 2 * big:
        return [m_per]
    return [big] * (m_per // big - 1) + [256, 128, 64, 32, 16, 16]


def _better(v, bv):
    return jnp.logical_and(jnp.logical_not(v <= bv), bv == bv)


def pallas_dist_argmax_global_i_m4096_n1024_kernel(x):
    m_per, n = x.shape
    chunks = _chunk_rows(m_per)
    offs = [sum(chunks[:c]) for c in range(len(chunks))]

    def body(x_hbm, out_ref, buf, comm, in_sems, send_sems, recv_sems):
        my = lax.axis_index("i")

        barrier = pltpu.get_barrier_semaphore()
        for d in range(1, N_DEV):
            pl.semaphore_signal(
                barrier, inc=1, device_id=((my + d) % N_DEV,),
                device_id_type=pl.DeviceIdType.MESH)

        def load(c):
            return pltpu.make_async_copy(
                x_hbm.at[pl.ds(offs[c], chunks[c])],
                buf.at[pl.ds(offs[c], chunks[c])], in_sems.at[c])

        for c in range(len(chunks)):
            load(c).start()

        def loop(g, carry):
            m, idx = carry
            xg = buf[pl.ds(pl.multiple_of(g * 8, 8), 8), :]
            gt = _better(xg, m)
            return jnp.where(gt, xg, m), jnp.where(gt, g, idx)

        m = jnp.full((8, n), -jnp.inf, jnp.float32)
        idx = jnp.zeros((8, n), jnp.int32)
        for c in range(len(chunks)):
            load(c).wait()
            g0 = offs[c] // 8
            m, idx = lax.fori_loop(g0, g0 + chunks[c] // 8, loop, (m, idx),
                                   unroll=min(UNROLL, chunks[c] // 8))

        rows = idx * 8 + lax.broadcasted_iota(jnp.int32, m.shape, 0)
        bv, br = m, rows
        for h in (4, 2, 1):
            v, r = bv[h:2 * h, :], br[h:2 * h, :]
            bv, br = bv[0:h, :], br[0:h, :]
            tie = jnp.logical_or(v == bv, jnp.logical_and(v != v, bv != bv))
            take = jnp.logical_or(_better(v, bv),
                                  jnp.logical_and(tie, r < br))
            bv, br = jnp.where(take, v, bv), jnp.where(take, r, br)
        comm[my, 0:1, :] = bv
        comm[my, 1:2, :] = (br + my * m_per).astype(jnp.float32)

        pl.semaphore_wait(barrier, N_DEV - 1)
        sends = []
        for d in range(1, N_DEV):
            cp = pltpu.make_async_remote_copy(
                src_ref=comm.at[my], dst_ref=comm.at[my],
                send_sem=send_sems.at[d - 1], recv_sem=recv_sems.at[d - 1],
                device_id=((my + d) % N_DEV,),
                device_id_type=pl.DeviceIdType.MESH)
            cp.start()
            sends.append(cp)
        for d in range(1, N_DEV):
            src = (my - d) % N_DEV
            pltpu.make_async_remote_copy(
                src_ref=comm.at[src], dst_ref=comm.at[src],
                send_sem=send_sems.at[d - 1], recv_sem=recv_sems.at[d - 1],
                device_id=(src,),
                device_id_type=pl.DeviceIdType.MESH).wait_recv()
        for cp in sends:
            cp.wait_send()

        bv, bi = comm[0, 0:1, :], comm[0, 1:2, :]
        for j in range(1, N_DEV):
            v = comm[j, 0:1, :]
            take = _better(v, bv)
            bi = jnp.where(take, comm[j, 1:2, :], bi)
            bv = jnp.where(take, v, bv)
        out_ref[0:1, :] = bv
        out_ref[1:2, :] = bi

    return pl.pallas_call(
        body,
        out_shape=jax.ShapeDtypeStruct((2, n), jnp.float32),
        in_specs=[pl.BlockSpec(memory_space=pl.ANY)],
        out_specs=pl.BlockSpec(memory_space=pltpu.VMEM),
        scratch_shapes=[
            pltpu.VMEM((m_per, n), jnp.float32),
            pltpu.VMEM((N_DEV, 2, n), jnp.float32),
            pltpu.SemaphoreType.DMA((len(chunks),)),
            pltpu.SemaphoreType.DMA((N_DEV - 1,)),
            pltpu.SemaphoreType.DMA((N_DEV - 1,)),
        ],
        compiler_params=pltpu.CompilerParams(
            collective_id=0, vmem_limit_bytes=64 * 1024 * 1024),
    )(x)
```
